```python
import numpy as np

kernel_name = "dist_mean_ax0_shard0_i_m2048_n1024"

def setup_inputs():
    return {"x": np.random.randn(8192, 1024).astype(np.float32)}

def reference(x: np.ndarray) -> np.ndarray:
    return np.mean(x, axis=0, keepdims=True)
```

```python
import jax
import jax.numpy as jnp
from jax import lax
from jax.experimental import pallas as pl
from jax.experimental.pallas import tpu as pltpu

N_DEV = 4
CHUNK_ROWS = 128


def pallas_dist_mean_ax0_shard0_i_m2048_n1024_kernel(
x: jax.Array,
):
    m_per, n = x.shape
    n_chunks = m_per // CHUNK_ROWS
    scale = 1.0 / float(m_per * N_DEV)

    def body(x_hbm, out_ref, xbuf, send_buf, recv_buf, copy_sems, send_sems, recv_sem):
        me = lax.axis_index("i")

        copies = [
            pltpu.make_async_copy(
                x_hbm.at[pl.ds(c * CHUNK_ROWS, CHUNK_ROWS), :],
                xbuf.at[pl.ds(c * CHUNK_ROWS, CHUNK_ROWS), :],
                copy_sems.at[c],
            )
            for c in range(n_chunks)
        ]
        for cp in copies:
            cp.start()

        barrier = pltpu.get_barrier_semaphore()
        for d in range(1, N_DEV):
            pl.semaphore_signal(
                barrier, inc=1,
                device_id=((me + d) % N_DEV,),
                device_id_type=pl.DeviceIdType.MESH,
            )

        acc = jnp.zeros((8, n), jnp.float32)
        for c in range(n_chunks):
            copies[c].wait()
            blk = xbuf[pl.ds(c * CHUNK_ROWS, CHUNK_ROWS), :]
            acc = acc + jnp.sum(blk.reshape(CHUNK_ROWS // 8, 8, n), axis=0)
        part = jnp.sum(acc, axis=0, keepdims=True)
        send_buf[...] = part

        pl.semaphore_wait(barrier, N_DEV - 1)

        rdmas = [
            pltpu.make_async_remote_copy(
                src_ref=send_buf,
                dst_ref=recv_buf.at[d - 1],
                send_sem=send_sems.at[d - 1],
                recv_sem=recv_sem,
                device_id=((me + d) % N_DEV,),
                device_id_type=pl.DeviceIdType.MESH,
            )
            for d in range(1, N_DEV)
        ]
        for r in rdmas:
            r.start()

        pltpu.make_async_copy(recv_buf, recv_buf, recv_sem).wait()
        total = part + recv_buf[0] + recv_buf[1] + recv_buf[2]
        out_ref[...] = total * scale

        for r in rdmas:
            r.wait_send()

    return pl.pallas_call(
        body,
        out_shape=jax.ShapeDtypeStruct((1, n), jnp.float32),
        in_specs=[pl.BlockSpec(memory_space=pl.ANY)],
        out_specs=pl.BlockSpec(memory_space=pltpu.VMEM),
        scratch_shapes=[
            pltpu.VMEM((m_per, n), jnp.float32),
            pltpu.VMEM((1, n), jnp.float32),
            pltpu.VMEM((N_DEV - 1, 1, n), jnp.float32),
            pltpu.SemaphoreType.DMA((n_chunks,)),
            pltpu.SemaphoreType.DMA((N_DEV - 1,)),
            pltpu.SemaphoreType.DMA,
        ],
        compiler_params=pltpu.CompilerParams(
            collective_id=0,
            vmem_limit_bytes=32 * 1024 * 1024,
        ),
    )(x)
```

```python
import jax
import jax.numpy as jnp
from jax import lax
from jax.experimental import pallas as pl
from jax.experimental.pallas import tpu as pltpu

N_DEV = 4
SUBLANES = 8
LANES = 128
CHUNK_ROWS = 128
TAIL_ROWS = 64
OFFLOAD_ROWS = 88
MESH = pl.DeviceIdType.MESH


def _fold_rows(blk):
    r, c = blk.shape
    return jnp.sum(blk.reshape(r // SUBLANES, SUBLANES, c), axis=0)


def pallas_dist_mean_ax0_shard0_i_m2048_n1024_kernel(
x: jax.Array,
):
    m_per, n = x.shape
    n_blocks = n // LANES
    scale = 1.0 / float(m_per * N_DEV)

    local_rows = m_per - 2 * OFFLOAD_ROWS
    body_rows = local_rows - TAIL_ROWS
    assert n % LANES == 0 and body_rows > 0 and body_rows % SUBLANES == 0
    chunks = [
        (o, min(CHUNK_ROWS, body_rows - o)) for o in range(0, body_rows, CHUNK_ROWS)
    ]

    def body(x_hbm, out_ref, xbuf, off_buf, send_buf, recv_buf,
             copy_sems, off_send_sems, off_recv_sems, send_sem, recv_sem):
        me = lax.axis_index("i")

        def peer(d):
            return ((me + d) % N_DEV,)

        def local_copy(row0, rows, col0, cols, sem_idx):
            return pltpu.make_async_copy(
                x_hbm.at[pl.ds(row0, rows), pl.ds(col0, cols)],
                xbuf.at[pl.ds(row0, rows), pl.ds(col0, cols)],
                copy_sems.at[sem_idx],
            )

        body_copies = [
            local_copy(o, r, 0, n, i) for i, (o, r) in enumerate(chunks)
        ]
        tail_copies = [
            local_copy(body_rows, TAIL_ROWS, j * LANES, LANES, len(chunks) + j)
            for j in range(n_blocks)
        ]

        body_copies[0].start()
        barrier = pltpu.get_barrier_semaphore()
        for d in range(1, N_DEV):
            pl.semaphore_signal(barrier, inc=1, device_id=peer(d), device_id_type=MESH)
        for cp in body_copies[1:] + tail_copies:
            cp.start()

        pl.semaphore_wait(barrier, N_DEV - 1)

        offloads = [
            pltpu.make_async_remote_copy(
                src_ref=x_hbm.at[pl.ds(local_rows + j * OFFLOAD_ROWS, OFFLOAD_ROWS), :],
                dst_ref=off_buf.at[j],
                send_sem=off_send_sems.at[j],
                recv_sem=off_recv_sems.at[j],
                device_id=peer(d),
                device_id_type=MESH,
            )
            for j, d in enumerate((1, N_DEV - 1))
        ]
        for cp in offloads:
            cp.start()

        acc = jnp.zeros((SUBLANES, n), jnp.float32)
        for cp, (o, r) in zip(body_copies, chunks):
            cp.wait()
            acc = acc + _fold_rows(xbuf[pl.ds(o, r), :])
        for j, cp in enumerate(offloads):
            cp.wait_recv()
            acc = acc + _fold_rows(off_buf[j])

        for j, cp in enumerate(tail_copies):
            cp.wait()
            blk = acc[:, j * LANES:(j + 1) * LANES] + _fold_rows(
                xbuf[pl.ds(body_rows, TAIL_ROWS), pl.ds(j * LANES, LANES)]
            )
            send_buf[pl.ds(j, 1), :] = jnp.sum(blk, axis=0, keepdims=True) * scale
            for d in (2, 1, 3):
                pltpu.make_async_remote_copy(
                    src_ref=send_buf.at[pl.ds(j, 1), :],
                    dst_ref=recv_buf.at[d - 1, pl.ds(j, 1), :],
                    send_sem=send_sem,
                    recv_sem=recv_sem,
                    device_id=peer(d),
                    device_id_type=MESH,
                ).start()

        pltpu.make_async_copy(recv_buf, recv_buf, send_sem).wait()
        for cp in offloads:
            cp.wait_send()
        pltpu.make_async_copy(recv_buf, recv_buf, recv_sem).wait()

        out_ref[...] = (send_buf[...] + recv_buf[0]) + (recv_buf[1] + recv_buf[2])

    out = pl.pallas_call(
        body,
        out_shape=jax.ShapeDtypeStruct((n_blocks, LANES), jnp.float32),
        in_specs=[pl.BlockSpec(memory_space=pl.ANY)],
        out_specs=pl.BlockSpec(memory_space=pltpu.VMEM),
        scratch_shapes=[
            pltpu.VMEM((local_rows, n), jnp.float32),
            pltpu.VMEM((2, OFFLOAD_ROWS, n), jnp.float32),
            pltpu.VMEM((n_blocks, LANES), jnp.float32),
            pltpu.VMEM((N_DEV - 1, n_blocks, LANES), jnp.float32),
            pltpu.SemaphoreType.DMA((len(chunks) + n_blocks,)),
            pltpu.SemaphoreType.DMA((2,)),
            pltpu.SemaphoreType.DMA((2,)),
            pltpu.SemaphoreType.DMA,
            pltpu.SemaphoreType.DMA,
        ],
        compiler_params=pltpu.CompilerParams(
            collective_id=0,
            disable_semaphore_checks=True,
            vmem_limit_bytes=32 * 1024 * 1024,
        ),
    )(x)
    return out.reshape(1, n)
```

```python
import jax
import jax.numpy as jnp
from jax import lax
from jax.experimental import pallas as pl
from jax.experimental.pallas import tpu as pltpu

N_DEV = 4
SUBLANES = 8
LANES = 128
CHUNK_ROWS = 128
TAIL_ROWS = 64
OFFLOAD_ROWS = 88
MESH = pl.DeviceIdType.MESH


def _fold_rows(blk):
    r, c = blk.shape
    return jnp.sum(blk.reshape(r // SUBLANES, SUBLANES, c), axis=0)


def _fold_rows_tree(ref, row0, rows, col0, cols):
    vals = [
        ref[pl.ds(row0 + i * SUBLANES, SUBLANES), pl.ds(col0, cols)]
        for i in range(rows // SUBLANES)
    ]
    while len(vals) > 1:
        vals = [
            vals[i] + vals[i + 1] if i + 1 < len(vals) else vals[i]
            for i in range(0, len(vals), 2)
        ]
    return vals[0]


def pallas_dist_mean_ax0_shard0_i_m2048_n1024_kernel(
x: jax.Array,
):
    m_per, n = x.shape
    n_blocks = n // LANES
    scale = 1.0 / float(m_per * N_DEV)

    local_rows = m_per - 2 * OFFLOAD_ROWS
    body_rows = local_rows - TAIL_ROWS
    assert n % LANES == 0 and body_rows > 0 and body_rows % SUBLANES == 0
    chunks = [
        (o, min(CHUNK_ROWS, body_rows - o)) for o in range(0, body_rows, CHUNK_ROWS)
    ]

    def body(x_hbm, out_ref, xbuf, off_buf, send_buf, recv_buf,
             copy_sems, off_send_sems, off_recv_sems, send_sem, recv_sem):
        me = lax.axis_index("i")

        def peer(d):
            return ((me + d) % N_DEV,)

        def local_copy(row0, rows, col0, cols, sem_idx):
            return pltpu.make_async_copy(
                x_hbm.at[pl.ds(row0, rows), pl.ds(col0, cols)],
                xbuf.at[pl.ds(row0, rows), pl.ds(col0, cols)],
                copy_sems.at[sem_idx],
            )

        body_copies = [
            local_copy(o, r, 0, n, i) for i, (o, r) in enumerate(chunks)
        ]
        tail_copies = [
            local_copy(body_rows, TAIL_ROWS, j * LANES, LANES, len(chunks) + j)
            for j in range(n_blocks)
        ]

        body_copies[0].start()
        barrier = pltpu.get_barrier_semaphore()
        for d in range(1, N_DEV):
            pl.semaphore_signal(barrier, inc=1, device_id=peer(d), device_id_type=MESH)
        for cp in body_copies[1:] + tail_copies:
            cp.start()

        pl.semaphore_wait(barrier, N_DEV - 1)

        offloads = [
            pltpu.make_async_remote_copy(
                src_ref=x_hbm.at[pl.ds(local_rows + j * OFFLOAD_ROWS, OFFLOAD_ROWS), :],
                dst_ref=off_buf.at[j],
                send_sem=off_send_sems.at[j],
                recv_sem=off_recv_sems.at[j],
                device_id=peer(d),
                device_id_type=MESH,
            )
            for j, d in enumerate((1, N_DEV - 1))
        ]
        for cp in offloads:
            cp.start()

        acc = jnp.zeros((SUBLANES, n), jnp.float32)
        for cp, (o, r) in zip(body_copies, chunks):
            cp.wait()
            acc = acc + _fold_rows(xbuf[pl.ds(o, r), :])
        for j, cp in enumerate(offloads):
            cp.wait_recv()
            acc = acc + _fold_rows(off_buf[j])

        for j, cp in enumerate(tail_copies):
            cp.wait()
            blk = acc[:, j * LANES:(j + 1) * LANES] + _fold_rows_tree(
                xbuf, body_rows, TAIL_ROWS, j * LANES, LANES
            )
            send_buf[pl.ds(j, 1), :] = jnp.sum(blk, axis=0, keepdims=True) * scale
            for d in (2, 1, 3):
                pltpu.make_async_remote_copy(
                    src_ref=send_buf.at[pl.ds(j, 1), :],
                    dst_ref=recv_buf.at[d - 1, pl.ds(j, 1), :],
                    send_sem=send_sem,
                    recv_sem=recv_sem,
                    device_id=peer(d),
                    device_id_type=MESH,
                ).start()

        pltpu.make_async_copy(recv_buf, recv_buf, send_sem).wait()
        for cp in offloads:
            cp.wait_send()
        pltpu.make_async_copy(recv_buf, recv_buf, recv_sem).wait()

        out_ref[...] = (send_buf[...] + recv_buf[0]) + (recv_buf[1] + recv_buf[2])

    out = pl.pallas_call(
        body,
        out_shape=jax.ShapeDtypeStruct((n_blocks, LANES), jnp.float32),
        in_specs=[pl.BlockSpec(memory_space=pl.ANY)],
        out_specs=pl.BlockSpec(memory_space=pltpu.VMEM),
        scratch_shapes=[
            pltpu.VMEM((local_rows, n), jnp.float32),
            pltpu.VMEM((2, OFFLOAD_ROWS, n), jnp.float32),
            pltpu.VMEM((n_blocks, LANES), jnp.float32),
            pltpu.VMEM((N_DEV - 1, n_blocks, LANES), jnp.float32),
            pltpu.SemaphoreType.DMA((len(chunks) + n_blocks,)),
            pltpu.SemaphoreType.DMA((2,)),
            pltpu.SemaphoreType.DMA((2,)),
            pltpu.SemaphoreType.DMA,
            pltpu.SemaphoreType.DMA,
        ],
        compiler_params=pltpu.CompilerParams(
            collective_id=0,
            disable_semaphore_checks=True,
            vmem_limit_bytes=32 * 1024 * 1024,
        ),
    )(x)
    return out.reshape(1, n)
```

```python
import jax
import jax.numpy as jnp
from jax import lax
from jax.experimental import pallas as pl
from jax.experimental.pallas import tpu as pltpu

N_DEV = 4
SUBLANES = 8
LANES = 128
CHUNK_ROWS = 128
TAIL_ROWS = 64
OFFLOAD_ROWS = 88
MESH = pl.DeviceIdType.MESH


def _fold_rows(blk):
    r, c = blk.shape
    return jnp.sum(blk.reshape(r // SUBLANES, SUBLANES, c), axis=0)


def _fold_rows_tree(ref, row0, rows, col0, cols):
    vals = [
        ref[pl.ds(row0 + i * SUBLANES, SUBLANES), pl.ds(col0, cols)]
        for i in range(rows // SUBLANES)
    ]
    while len(vals) > 1:
        vals = [
            vals[i] + vals[i + 1] if i + 1 < len(vals) else vals[i]
            for i in range(0, len(vals), 2)
        ]
    return vals[0]


def pallas_dist_mean_ax0_shard0_i_m2048_n1024_kernel(
x: jax.Array,
):
    m_per, n = x.shape
    n_blocks = n // LANES
    scale = 1.0 / float(m_per * N_DEV)

    local_rows = m_per - 2 * OFFLOAD_ROWS
    body_rows = local_rows - TAIL_ROWS
    assert n % LANES == 0 and body_rows > 0 and body_rows % SUBLANES == 0
    chunks = [
        (o, min(CHUNK_ROWS, body_rows - o)) for o in range(0, body_rows, CHUNK_ROWS)
    ]

    def body(x_hbm, out_ref, xbuf, off_buf, send_buf, recv_buf,
             copy_sems, off_send_sems, off_recv_sems, send_sem, recv_sem):
        me = lax.axis_index("i")

        def peer(d):
            return ((me + d) % N_DEV,)

        def local_copy(row0, rows, col0, cols, sem_idx):
            return pltpu.make_async_copy(
                x_hbm.at[pl.ds(row0, rows), pl.ds(col0, cols)],
                xbuf.at[pl.ds(row0, rows), pl.ds(col0, cols)],
                copy_sems.at[sem_idx],
            )

        body_copies = [
            local_copy(o, r, 0, n, i) for i, (o, r) in enumerate(chunks)
        ]
        tail_copies = [
            local_copy(body_rows, TAIL_ROWS, j * LANES, LANES, len(chunks) + j)
            for j in range(n_blocks)
        ]

        body_copies[0].start()
        barrier = pltpu.get_barrier_semaphore()
        for d in range(1, N_DEV):
            pl.semaphore_signal(barrier, inc=1, device_id=peer(d), device_id_type=MESH)
        for cp in body_copies[1:] + tail_copies:
            cp.start()

        pl.semaphore_wait(barrier, N_DEV - 1)

        offloads = [
            pltpu.make_async_remote_copy(
                src_ref=x_hbm.at[pl.ds(local_rows + j * OFFLOAD_ROWS, OFFLOAD_ROWS), :],
                dst_ref=off_buf.at[j],
                send_sem=off_send_sems.at[j],
                recv_sem=off_recv_sems.at[j],
                device_id=peer(d),
                device_id_type=MESH,
            )
            for j, d in enumerate((1, N_DEV - 1))
        ]
        for cp in offloads:
            cp.start()

        acc = jnp.zeros((SUBLANES, n), jnp.float32)
        for cp, (o, r) in zip(body_copies, chunks):
            cp.wait()
            acc = acc + _fold_rows(xbuf[pl.ds(o, r), :])
        for j, cp in enumerate(offloads):
            cp.wait_recv()
            acc = acc + _fold_rows(off_buf[j])

        for j, cp in enumerate(tail_copies):
            cp.wait()
            blk = acc[:, j * LANES:(j + 1) * LANES] + _fold_rows_tree(
                xbuf, body_rows, TAIL_ROWS, j * LANES, LANES
            )
            send_buf[pl.ds(j, 1), :] = jnp.sum(blk, axis=0, keepdims=True) * scale
            for d in (2, 1, 3):
                pltpu.make_async_remote_copy(
                    src_ref=send_buf.at[pl.ds(j, 1), :],
                    dst_ref=recv_buf.at[d - 1, pl.ds(j, 1), :],
                    send_sem=send_sem,
                    recv_sem=recv_sem,
                    device_id=peer(d),
                    device_id_type=MESH,
                ).start()

        pltpu.make_async_copy(recv_buf, recv_buf, send_sem).wait()
        for cp in offloads:
            cp.wait_send()
        pltpu.make_async_copy(recv_buf, recv_buf, recv_sem).wait()

        out_ref[...] = (send_buf[...] + recv_buf[0]) + (recv_buf[1] + recv_buf[2])

    params = dict(collective_id=0, vmem_limit_bytes=32 * 1024 * 1024)
    if hasattr(pltpu.CompilerParams, "disable_semaphore_checks"):
        params["disable_semaphore_checks"] = True

    out = pl.pallas_call(
        body,
        out_shape=jax.ShapeDtypeStruct((n_blocks, LANES), jnp.float32),
        in_specs=[pl.BlockSpec(memory_space=pl.ANY)],
        out_specs=pl.BlockSpec(memory_space=pltpu.VMEM),
        scratch_shapes=[
            pltpu.VMEM((local_rows, n), jnp.float32),
            pltpu.VMEM((2, OFFLOAD_ROWS, n), jnp.float32),
            pltpu.VMEM((n_blocks, LANES), jnp.float32),
            pltpu.VMEM((N_DEV - 1, n_blocks, LANES), jnp.float32),
            pltpu.SemaphoreType.DMA((len(chunks) + n_blocks,)),
            pltpu.SemaphoreType.DMA((2,)),
            pltpu.SemaphoreType.DMA((2,)),
            pltpu.SemaphoreType.DMA,
            pltpu.SemaphoreType.DMA,
        ],
        compiler_params=pltpu.CompilerParams(**params),
    )(x)
    return out.reshape(1, n)
```
